```python
import numpy as np

kernel_name = "dist_mean_ax1_xy_m4096_n1024"

def setup_inputs():
    return {"x": np.random.randn(8192, 2048).astype(np.float32)}

def reference(x: np.ndarray) -> np.ndarray:
    return np.mean(x, axis=1, keepdims=True)
```

```python
import jax
import jax.numpy as jnp
from jax import lax
from jax.experimental import pallas as pl
from jax.experimental.pallas import tpu as pltpu

LANES = 128
CHUNK = 256


def pallas_dist_mean_ax1_xy_m4096_n1024_kernel(
x: jax.Array,
):
    m, n = x.shape
    n_chunks = m // CHUNK
    groups = m // LANES
    scale = 1.0 / (2 * n)

    def kernel_body(x_hbm, out_ref, xbuf, mine, theirs, load_sems, send_sem, recv_sem):
        my_x = lax.axis_index("x")
        my_y = lax.axis_index("y")
        peer = (my_x, 1 - my_y)

        def load(c):
            rows = pl.ds(c * CHUNK, CHUNK)
            return pltpu.make_async_copy(x_hbm.at[rows], xbuf.at[rows], load_sems.at[c])

        for c in range(n_chunks):
            load(c).start()

        barrier = pltpu.get_barrier_semaphore()
        pl.semaphore_signal(barrier, inc=1, device_id=peer,
                            device_id_type=pl.DeviceIdType.MESH)

        for c in range(n_chunks):
            load(c).wait()
            for g in range(CHUNK // LANES):
                r0 = c * CHUNK + g * LANES
                acc = xbuf[pl.ds(r0, LANES), pl.ds(0, LANES)]
                for j in range(1, n // LANES):
                    acc = acc + xbuf[pl.ds(r0, LANES), pl.ds(j * LANES, LANES)]
                row = jnp.sum(acc.T, axis=0, keepdims=True)
                mine[pl.ds(r0 // LANES, 1), :] = row

        pl.semaphore_wait(barrier, 1)
        rdma = pltpu.make_async_remote_copy(
            mine, theirs, send_sem, recv_sem, device_id=peer,
            device_id_type=pl.DeviceIdType.MESH)
        rdma.start()
        rdma.wait()
        out_ref[...] = (mine[...] + theirs[...]) * scale

    out = pl.pallas_call(
        kernel_body,
        out_shape=jax.ShapeDtypeStruct((groups, LANES), jnp.float32),
        in_specs=[pl.BlockSpec(memory_space=pltpu.HBM)],
        out_specs=pl.BlockSpec(memory_space=pltpu.VMEM),
        scratch_shapes=[
            pltpu.VMEM((m, n), jnp.float32),
            pltpu.VMEM((groups, LANES), jnp.float32),
            pltpu.VMEM((groups, LANES), jnp.float32),
            pltpu.SemaphoreType.DMA((n_chunks,)),
            pltpu.SemaphoreType.DMA,
            pltpu.SemaphoreType.DMA,
        ],
        compiler_params=pltpu.CompilerParams(
            collective_id=0, vmem_limit_bytes=48 * 1024 * 1024),
    )(x)
    return out.reshape(m, 1)
```

```python
import jax
import jax.numpy as jnp
from jax import lax
from jax.experimental import pallas as pl
from jax.experimental.pallas import tpu as pltpu

LANES = 128
SUBLANES = 8

HEAD_GROUPS = 3
Y_TILES = 232
BLOCK_SHIFT = 9
LONG_SWEEPS = 5
BULK_GROUPS = 21
LAST_STRIPS = 3

HEAD, BULK, REST, TAIL = range(4)


def pallas_dist_mean_ax1_xy_m4096_n1024_kernel(
    x: jax.Array,
):
    m, n = x.shape
    strip = n // LANES
    group = LANES // SUBLANES * strip
    block = 2 * strip
    n_tiles = m // SUBLANES * strip
    n_groups = m // LANES
    n_sweeps = group // block
    last_group = n_groups - 1
    head_end = HEAD_GROUPS * group - BLOCK_SHIFT
    tail_start = last_group * group - BLOCK_SHIFT + LONG_SWEEPS * block
    tail_split = n_tiles - LAST_STRIPS * strip
    parts = (
        (0, HEAD_GROUPS),
        (HEAD_GROUPS, HEAD_GROUPS + BULK_GROUPS),
        (HEAD_GROUPS + BULK_GROUPS, last_group),
        (last_group, n_groups),
    )
    scale = 1.0 / (2 * n)

    def kernel_body(
        x_hbm, out_ref,
        tiles, handed, strip_sums, side_out, side_in, mine, theirs,
        sweep_sems, span_sems, part_send, part_recv,
        raw_send, raw_recv, side_send, side_recv, go,
    ):
        my_x = lax.axis_index("x")
        my_y = lax.axis_index("y")
        peer = (my_x, 1 - my_y)
        across = (1 - my_x, my_y)
        diagonal = (1 - my_x, 1 - my_y)
        early = my_y == 0
        late = my_y == 1

        def load(start, size, sem):
            span = pl.ds(start, size)
            return pltpu.make_async_copy(x_hbm.at[span], tiles.at[span], sem)

        def block_load(p, g, sem):
            return load(g * group + p * block - BLOCK_SHIFT, block, sweep_sems.at[sem])

        def start_sweep(p, lo, hi, sem):
            @pl.loop(lo, hi)
            def _(g):
                block_load(p, g, sem).start()

        def wait_sweep(p, lo, hi):
            @pl.loop(lo, hi)
            def _(g):
                block_load(p, g, p).wait()

        def sweep_end(p):
            return jnp.where(p < LONG_SWEEPS, n_groups, last_group)

        def head_load():
            return load(0, head_end, span_sems.at[0])

        def tail_load():
            return load(tail_start, tail_split - tail_start, span_sems.at[1])

        def last_load():
            return load(tail_split, n_tiles - tail_split, span_sems.at[2])

        def remote_copy(src, dst, send_sem, recv_sem, to):
            return pltpu.make_async_remote_copy(
                src, dst, send_sem, recv_sem,
                device_id=to, device_id_type=pl.DeviceIdType.MESH)

        def raw(lo, hi, i, to):
            span = pl.ds(lo, hi - lo)
            return remote_copy(x_hbm.at[span], handed.at[span], raw_send.at[i], raw_recv, to)

        def raw_y():
            return raw(0, Y_TILES, 0, peer)

        def raw_x():
            return raw(Y_TILES, head_end, 1, across)

        def side(i):
            return remote_copy(
                side_out, side_in, side_send.at[i], side_recv, (across, diagonal)[i])

        def part(i):
            return remote_copy(mine[i], theirs[i], part_send.at[i], part_recv.at[i], peer)

        def signal(sem, to):
            pl.semaphore_signal(sem, inc=1, device_id=to, device_id_type=pl.DeviceIdType.MESH)

        start_sweep(0, HEAD_GROUPS, HEAD_GROUPS + 2, 0)
        barrier = pltpu.get_barrier_semaphore()
        signal(barrier, peer)

        @pl.when(late)
        def _():
            signal(barrier, diagonal)
            pl.semaphore_wait(barrier, 1)
            raw_y().start()

        start_sweep(0, HEAD_GROUPS + 2, n_groups, 0)
        start_sweep(1, HEAD_GROUPS, sweep_end(1), 1)

        @pl.when(early)
        def _():
            pl.semaphore_wait(barrier, 2)
            signal(go, peer)
            signal(go, diagonal)
            head_load().start()

        @pl.when(late)
        def _():
            pl.semaphore_wait(go, 2)
            raw_x().start()

        lane = lax.broadcasted_iota(jnp.int32, (SUBLANES, LANES), 1)
        offset = lane - lax.broadcasted_iota(jnp.int32, (SUBLANES, LANES), 0)
        zeros = jnp.zeros((SUBLANES, LANES), jnp.float32)

        def row_sums(ref, ts):
            vs = [ref[t] for t in ts]
            while len(vs) > 1:
                vs = [a + b for a, b in zip(vs[::2], vs[1::2])] + vs[len(vs) // 2 * 2:]
            return jnp.sum(vs[0], axis=1, keepdims=True)

        def place(acc, ref, g, lo, hi):
            for j in range(group // strip):
                t = g * group + j * strip
                ts = range(max(t, lo), min(t + strip, hi))
                if ts:
                    acc = jnp.where(offset == j * SUBLANES, row_sums(ref, ts), acc)
            return acc

        def group_row(ref, g, lo, hi):
            return jnp.sum(place(zeros, ref, g, lo, hi), axis=0, keepdims=True)

        def reduce_strips(k, lo, hi):
            first = lane // SUBLANES == 2 * k
            both = lane // (2 * SUBLANES) == k
            for g in range(lo, hi):
                ts = [k * block + (g * group + c) for c in range(block)]
                sums = jnp.where(first, row_sums(tiles, ts[:strip]), row_sums(tiles, ts[strip:]))
                pltpu.store(strip_sums.at[pl.ds(g * SUBLANES, SUBLANES)], sums, mask=both)

        def collect(i):
            lo, hi = parts[i]
            for g in range(lo, hi, SUBLANES):
                rows = strip_sums[pl.ds(g * SUBLANES, SUBLANES, stride=SUBLANES), :]
                for r in range(1, SUBLANES):
                    rows = jnp.where(
                        lane % SUBLANES == r,
                        strip_sums[pl.ds(g * SUBLANES + r, SUBLANES, stride=SUBLANES), :],
                        rows)
                count = min(SUBLANES, hi - g)
                mine[i][pl.ds(g - lo, count), :] = rows[:count]

        strip_sums[...] = jnp.zeros(strip_sums.shape, jnp.float32)
        wait_sweep(0, HEAD_GROUPS, n_groups)

        @pl.loop(0, n_sweeps - 2)
        def _(k):
            @pl.when(k < n_sweeps - 3)
            def _():
                start_sweep(k + 2, HEAD_GROUPS, sweep_end(k + 2), k + 2)

            @pl.when(k == n_sweeps - 3)
            def _():
                start_sweep(n_sweeps - 1, *parts[BULK], n_sweeps - 1)
                start_sweep(n_sweeps - 1, *parts[REST], n_sweeps)

            wait_sweep(k + 1, HEAD_GROUPS, sweep_end(k + 1))
            reduce_strips(k, HEAD_GROUPS, last_group)

        tail_load().start()
        last_load().start()

        @pl.when(late)
        def _():
            for g in range(HEAD_GROUPS):
                mine[HEAD][pl.ds(g, 1), :] = group_row(tiles, g, head_end, n_tiles)
            part(HEAD).start()
            raw_x().wait_recv()
            for g in range(HEAD_GROUPS):
                side_out[pl.ds(g, 1), :] = group_row(handed, g, Y_TILES, head_end)
            side(0).start()
            side(1).start()

        ready = tail_start // strip * strip
        acc = place(zeros, tiles, last_group, 0, ready)
        for i, sem in ((BULK, n_sweeps - 1), (REST, n_sweeps)):
            for g in range(*parts[i]):
                block_load(n_sweeps - 1, g, sem).wait()
            reduce_strips(n_sweeps - 2, *parts[i])
            reduce_strips(n_sweeps - 1, *parts[i])
            collect(i)
            part(i).start()

        tail_load().wait()
        acc = place(acc, tiles, last_group, ready, tail_split)
        last_load().wait()
        acc = place(acc, tiles, last_group, tail_split, n_tiles)
        mine[TAIL][...] = jnp.sum(acc, axis=0, keepdims=True)
        part(TAIL).start()

        @pl.when(early)
        def _():
            head_load().wait()
            for g in range(HEAD_GROUPS):
                mine[HEAD][pl.ds(g, 1), :] = group_row(tiles, g, 0, n_tiles)
            raw_y().wait_recv()
            for g in range(pl.cdiv(Y_TILES, group)):
                mine[HEAD][pl.ds(g, 1), :] += group_row(handed, g, 0, Y_TILES)
            part(HEAD).start()
            side(1).wait_recv()

        @pl.when(late)
        def _():
            side(0).wait_recv()
            for copy in (raw_y(), raw_x(), side(0), side(1)):
                copy.wait_send()

        def finish(i):
            part(i).wait_recv()
            total = mine[i][...] + theirs[i][...]
            if i == HEAD:
                total += side_in[...]
            lo, hi = parts[i]
            out_ref[pl.ds(lo, hi - lo), :] = total * scale

        for i in (HEAD, BULK, REST):
            finish(i)
        for i in (HEAD, BULK, REST, TAIL):
            part(i).wait_send()
        finish(TAIL)

    def vmem(*shape):
        return pltpu.VMEM(shape, jnp.float32)

    dma = pltpu.SemaphoreType.DMA
    part_rows = [vmem(hi - lo, LANES) for lo, hi in parts]
    x_tiles = x.reshape(m // SUBLANES, SUBLANES, strip, LANES).transpose(0, 2, 1, 3)
    out = pl.pallas_call(
        kernel_body,
        out_shape=jax.ShapeDtypeStruct((n_groups, LANES), jnp.float32),
        in_specs=[pl.BlockSpec(memory_space=pltpu.HBM)],
        out_specs=pl.BlockSpec(memory_space=pltpu.VMEM),
        scratch_shapes=[
            vmem(n_tiles, SUBLANES, LANES),
            vmem(head_end, SUBLANES, LANES),
            vmem((n_groups + SUBLANES) * SUBLANES, LANES),
            vmem(HEAD_GROUPS, LANES),
            vmem(HEAD_GROUPS, LANES),
            part_rows,
            part_rows,
            dma((n_sweeps + 1,)),
            dma((3,)),
            dma((len(parts),)),
            dma((len(parts),)),
            dma((2,)),
            dma,
            dma((2,)),
            dma,
            pltpu.SemaphoreType.REGULAR,
        ],
        compiler_params=pltpu.CompilerParams(
            collective_id=0,
            vmem_limit_bytes=32 * 1024 * 1024,
            disable_semaphore_checks=True,
        ),
    )(x_tiles.reshape(n_tiles, SUBLANES, LANES))
    return out.reshape(m, 1)
```
